```python
import numpy as np

kernel_name = "dist_mean_ax1_xy_m4096_n1024"

def setup_inputs():
    return {"x": np.random.randn(8192, 2048).astype(np.float32)}

def reference(x: np.ndarray) -> np.ndarray:
    return np.mean(x, axis=1, keepdims=True)
```

```python
import jax
import jax.numpy as jnp
from jax import lax
from jax.experimental import pallas as pl
from jax.experimental.pallas import tpu as pltpu

_LANES = 128
_SUBLANES = 8
_Y = 2

_BOUNDS = (0, 2048, 3584, 3840, 3880, 3888)
_UNROLL = 4


def pallas_dist_mean_ax1_xy_m4096_n1024_kernel(
x: jax.Array,
):
    m, n = x.shape
    groups = m // _LANES
    n_local = len(_BOUNDS) - 1
    pushed = pl.ds(_BOUNDS[-1], m - _BOUNDS[-1])
    scale = 1.0 / (_Y * n)

    def kernel_body(x_hbm, o_ref, xbuf, part, recv, in_sems, raw_sems, send_sems, recv_sems):
        def load(c):
            rows = pl.ds(_BOUNDS[c], _BOUNDS[c + 1] - _BOUNDS[c])
            return pltpu.make_async_copy(x_hbm.at[rows], xbuf.at[rows], in_sems.at[c])

        load(0).start()
        peer = (lax.axis_index("x"), 1 - lax.axis_index("y"))
        barrier = pltpu.get_barrier_semaphore()
        pl.semaphore_signal(barrier, inc=1, device_id=peer, device_id_type=pl.DeviceIdType.MESH)
        for c in range(1, n_local):
            load(c).start()
        pl.semaphore_wait(barrier, 1)
        raw = pltpu.make_async_remote_copy(
            x_hbm.at[pushed], xbuf.at[pushed], raw_sems.at[0], raw_sems.at[1],
            device_id=peer, device_id_type=pl.DeviceIdType.MESH)
        raw.start()

        tile = (_SUBLANES, _LANES)
        diag = lax.broadcasted_iota(jnp.int32, tile, 1) - lax.broadcasted_iota(jnp.int32, tile, 0)

        def add_rows(acc, base, r0, r1):
            for r in range(r0, r1, _SUBLANES):
                v = [xbuf[pl.ds(base + r, _SUBLANES), pl.ds(k, _LANES)] for k in range(0, n, _LANES)]
                while len(v) > 1:
                    v = [v[i] + v[i + 1] for i in range(0, len(v), 2)]
                acc = jnp.where(diag == r, jnp.sum(v[0], axis=1, keepdims=True), acc)
            return acc

        def finish(g, acc):
            part[pl.ds(g, 1), :] = jnp.sum(acc, axis=0, keepdims=True) * scale

        zero = jnp.zeros(tile, jnp.float32)

        def reduce_groups(g0, g1):
            if g1 - g0 <= _UNROLL:
                for g in range(g0, g1):
                    finish(g, add_rows(zero, g * _LANES, 0, _LANES))
                return

            @pl.loop(0, (g1 - g0) // _UNROLL)
            def _(i):
                for u in range(_UNROLL):
                    g = g0 + i * _UNROLL + u
                    finish(g, add_rows(zero, pl.multiple_of(g * _LANES, _LANES), 0, _LANES))

        def send(i, g0, g1):
            rows = pl.ds(g0, g1 - g0)
            copy = pltpu.make_async_remote_copy(
                part.at[rows], recv.at[rows], send_sems.at[i], recv_sems.at[i],
                device_id=peer, device_id_type=pl.DeviceIdType.MESH)
            copy.start()
            return rows, copy

        sends = []
        load(0).wait()
        reduce_groups(0, 16)
        load(1).wait()
        reduce_groups(16, 28)
        sends.append(send(0, 0, 28))
        raw.wait_recv()
        acc = add_rows(zero, 30 * _LANES, _BOUNDS[-1] % _LANES, _LANES)
        reduce_groups(31, 32)
        load(2).wait()
        reduce_groups(28, 30)
        sends.append(send(1, 28, 30))
        sends.append(send(2, 31, 32))
        load(3).wait()
        acc = add_rows(acc, 30 * _LANES, _BOUNDS[3] % _LANES, _BOUNDS[4] % _LANES)
        load(4).wait()
        acc = add_rows(acc, 30 * _LANES, _BOUNDS[4] % _LANES, _BOUNDS[5] % _LANES)
        finish(30, acc)
        sends.append(send(3, 30, 31))

        raw.wait_send()
        for rows, copy in sends:
            copy.wait_send()
        for rows, copy in sends:
            copy.wait_recv()
            o_ref[rows, :] = part[rows, :] + recv[rows, :]

    out = pl.pallas_call(
        kernel_body,
        out_shape=jax.ShapeDtypeStruct((groups, _LANES), jnp.float32),
        in_specs=[pl.BlockSpec(memory_space=pltpu.HBM)],
        out_specs=pl.BlockSpec(memory_space=pltpu.VMEM),
        scratch_shapes=[
            pltpu.VMEM((m, n), jnp.float32),
            pltpu.VMEM((groups, _LANES), jnp.float32),
            pltpu.VMEM((groups, _LANES), jnp.float32),
            pltpu.SemaphoreType.DMA((n_local,)),
            pltpu.SemaphoreType.DMA((2,)),
            pltpu.SemaphoreType.DMA((4,)),
            pltpu.SemaphoreType.DMA((4,)),
        ],
        compiler_params=pltpu.CompilerParams(
            collective_id=0,
            vmem_limit_bytes=32 * 1024 * 1024,
            disable_bounds_checks=True,
            disable_semaphore_checks=True,
        ),
    )(x)
    return out.reshape(m, 1)
```

```python
import jax
import jax.numpy as jnp
from jax import lax
from jax.experimental import pallas as pl
from jax.experimental.pallas import tpu as pltpu

_SUBLANES = 8
_LANES = 128
_Y = 2
_UNROLL = 4

_HEAD = (0, 1024, 2048, 3072)
_TAIL_Y0 = (3072, 3840, 4096)
_TAIL_Y1 = (3072, 3328, 3488, 3512, 3528, 3536)
_LATE = _TAIL_Y1[2]
_VIA_SMEM = (3536, 3608, 3656)
_VIA_X = (3656, 3856)
_VIA_Y = (3856, 4096)


def _span(bounds, i=0, base=0):
    return pl.ds(bounds[i] - base, bounds[i + 1] - bounds[i])


def pallas_dist_mean_ax1_xy_m4096_n1024_kernel(
x: jax.Array,
):
    m, n = x.shape
    assert m == _VIA_Y[1] and n % _LANES == 0
    scale = 1.0 / (_Y * n)
    groups = m // _LANES
    g_tail = _HEAD[-1] // _LANES
    g_late = _LATE // _LANES
    g_x0, g_x1 = _VIA_X[0] // _LANES, pl.cdiv(_VIA_X[1], _LANES)
    g_y0 = _VIA_Y[0] // _LANES
    assert g_x0 == g_late + 1 and (_TAIL_Y1[-1] - 1) // _LANES == g_late

    def kernel_body(
        x_hbm, o_ref,
        x_vmem, y_vmem, x_smem, mine, theirs, x_sums, x_back, late_sums, late_smem,
        head_sems, tail_sems, smem_in_sems, smem_out_sems, send_sems, recv_sems, x_ready,
    ):
        def load(bounds, i, sems):
            rows = _span(bounds, i)
            return pltpu.make_async_copy(x_hbm.at[rows], x_vmem.at[rows], sems.at[i])

        head = [load(_HEAD, i, head_sems) for i in range(len(_HEAD) - 1)]
        head[0].start()

        my_x, my_y = lax.axis_index("x"), lax.axis_index("y")
        y_peer, x_peer = (my_x, 1 - my_y), (1 - my_x, my_y)
        barrier = pltpu.get_barrier_semaphore()

        def signal(sem, peer):
            pl.semaphore_signal(sem, inc=1, device_id=peer, device_id_type=pl.DeviceIdType.MESH)

        signal(barrier, y_peer)

        def remote(src, dst, i, peer):
            return pltpu.make_async_remote_copy(
                src, dst, send_sems.at[i], recv_sems.at[i],
                device_id=peer, device_id_type=pl.DeviceIdType.MESH)

        def sums_copy(i, g0, g1):
            rows = pl.ds(g0, g1 - g0)
            return remote(mine.at[rows], theirs.at[rows], i, y_peer)

        def late_copy():
            return remote(late_sums, late_smem, 4, y_peer)

        def rows_to_y_peer():
            return remote(x_hbm.at[_span(_VIA_Y)], y_vmem, 5, y_peer)

        def rows_to_x_peer():
            return remote(x_hbm.at[_span(_VIA_X)], x_vmem.at[_span(_VIA_X)], 6, x_peer)

        def sums_to_x_peer():
            return remote(x_sums, x_back, 7, x_peer)

        def smem_in(i):
            return pltpu.make_async_copy(
                x_hbm.at[_span(_VIA_SMEM, i)], x_smem.at[_span(_VIA_SMEM, i, _VIA_SMEM[0])],
                smem_in_sems.at[i])

        def smem_out(i):
            return pltpu.make_async_copy(
                x_smem.at[_span(_VIA_SMEM, i, _VIA_SMEM[0])], x_vmem.at[_span(_VIA_SMEM, i)],
                smem_out_sems.at[i])

        tile = (_SUBLANES, _LANES)
        diagonal = lax.broadcasted_iota(jnp.int32, tile, 1) - lax.broadcasted_iota(jnp.int32, tile, 0)
        zero = jnp.zeros(tile, jnp.float32)

        def fold(ref, r):
            v = [ref[pl.ds(r, _SUBLANES), pl.ds(c, _LANES)] for c in range(0, n, _LANES)]
            while len(v) > 1:
                v = [v[i] + v[i + 1] for i in range(0, len(v) - 1, 2)] + v[len(v) // 2 * 2:]
            return v[0]

        def place(acc, r, folded):
            return jnp.where(diagonal == r % _LANES, jnp.sum(folded, axis=1, keepdims=True), acc)

        def add_rows(acc, ref, r0, r1, offset=0):
            for r in range(r0, r1, _SUBLANES):
                acc = place(acc, r, fold(ref, offset + r))
            return acc

        def dense(acc):
            return jnp.sum(acc, axis=0, keepdims=True) * scale

        def overlap(g, r0, r1):
            return max(r0, g * _LANES), min(r1, (g + 1) * _LANES)

        def sum_groups(g0, g1):
            steps = (g1 - g0) // _UNROLL
            if steps > 1:
                @pl.loop(0, steps)
                def _(i):
                    for u in range(_UNROLL):
                        g = g0 + i * _UNROLL + u
                        start = pl.multiple_of(g * _LANES, _LANES)
                        mine[pl.ds(g, 1), :] = dense(add_rows(zero, x_vmem, 0, _LANES, start))
            for g in range(g0 + steps * _UNROLL if steps > 1 else g0, g1):
                mine[pl.ds(g, 1), :] = dense(add_rows(zero, x_vmem, 0, _LANES, g * _LANES))

        def finish(copy_index, g0, g1):
            sums_copy(copy_index, g0, g1).wait_recv()
            rows = pl.ds(g0, g1 - g0)
            o_ref[rows, :] = mine[rows, :] + theirs[rows, :]

        @pl.when(my_y == 1)
        def _():
            smem_in(0).start()

            @pl.when(my_x == 0)
            def _():
                signal(barrier, x_peer)
                pl.semaphore_wait(barrier, 1)

            @pl.when(my_x == 1)
            def _():
                pl.semaphore_wait(barrier, 2)
                signal(x_ready, x_peer)

            rows_to_y_peer().start()
            for copy in head[1:]:
                copy.start()
            for i in range(len(_TAIL_Y1) - 1):
                load(_TAIL_Y1, i, tail_sems).start()

            @pl.when(my_x == 0)
            def _():
                pl.semaphore_wait(x_ready, 1)

            rows_to_x_peer().start()

        @pl.when(my_y == 0)
        def _():
            for copy in head[1:]:
                copy.start()
            for i in range(len(_TAIL_Y0) - 1):
                load(_TAIL_Y0, i, tail_sems).start()
            pl.semaphore_wait(barrier, 1)

        smem_steps = len(_VIA_SMEM) - 1
        for i, copy in enumerate(head):
            copy.wait()
            if i < smem_steps:
                @pl.when(my_y == 1)
                def _():
                    smem_in(i).wait()
                    smem_out(i).start()
                    if i + 1 < smem_steps:
                        smem_in(i + 1).start()
            sum_groups(_HEAD[i] // _LANES, _HEAD[i + 1] // _LANES)
        sums_copy(0, 0, g_tail).start()

        @pl.when(my_y == 1)
        def _():
            rows_to_x_peer().wait_recv()
            for g in range(g_x0, g_x1):
                x_sums[pl.ds(g - g_x0, 1), :] = dense(add_rows(zero, x_vmem, *overlap(g, *_VIA_X)))
            sums_to_x_peer().start()

            load(_TAIL_Y1, 0, tail_sems).wait()
            sum_groups(g_tail, _TAIL_Y1[1] // _LANES)

            for i in range(smem_steps):
                smem_out(i).wait()
            acc = add_rows(zero, x_vmem, *overlap(g_late, _VIA_SMEM[0], _VIA_SMEM[-1]))
            for g in range(g_late + 1, groups):
                rows = overlap(g, _VIA_SMEM[0], _VIA_SMEM[-1])
                mine[pl.ds(g, 1), :] = dense(add_rows(zero, x_vmem, *rows))

            load(_TAIL_Y1, 1, tail_sems).wait()
            sum_groups(_TAIL_Y1[1] // _LANES, g_late)
            acc = add_rows(acc, x_vmem, g_late * _LANES, _LATE)
            sums_copy(1, g_tail, g_late).start()
            mine[pl.ds(g_late, 1), :] = dense(acc)
            sums_copy(3, g_late, g_late + 1).start()

            sums_to_x_peer().wait_recv()
            mine[pl.ds(g_x0, g_x1 - g_x0), :] += x_back[...]
            sums_copy(2, g_x0, g_x1).start()

            folded = []
            for i in range(2, len(_TAIL_Y1) - 1):
                load(_TAIL_Y1, i, tail_sems).wait()
                folded += [(r, fold(x_vmem, r)) for r in range(_TAIL_Y1[i], _TAIL_Y1[i + 1], _SUBLANES)]
            acc = zero
            for r, v in folded:
                acc = place(acc, r, v)
            late_sums[...] = dense(acc)
            late_copy().start()

            for copy in (
                rows_to_y_peer(), rows_to_x_peer(), sums_to_x_peer(), late_copy(),
                sums_copy(0, 0, g_tail), sums_copy(1, g_tail, g_late),
                sums_copy(2, g_x0, g_x1), sums_copy(3, g_late, g_late + 1),
            ):
                copy.wait_send()
            finish(0, 0, g_tail)
            finish(1, g_tail, groups)
            o_ref[pl.ds(g_late, 1), :] += late_sums[...]

        @pl.when(my_y == 0)
        def _():
            for i in range(len(_TAIL_Y0) - 1):
                load(_TAIL_Y0, i, tail_sems).wait()
                sum_groups(_TAIL_Y0[i] // _LANES, _TAIL_Y0[i + 1] // _LANES)

            rows_to_y_peer().wait_recv()
            for g in range(g_y0, groups):
                mine[pl.ds(g, 1), :] += dense(add_rows(zero, y_vmem, *overlap(g, *_VIA_Y), -_VIA_Y[0]))
            sums_copy(1, g_tail, groups).start()

            o_ref[pl.ds(g_x1, groups - g_x1), :] = mine[pl.ds(g_x1, groups - g_x1), :]
            finish(0, 0, g_tail)
            finish(1, g_tail, g_late)
            finish(2, g_x0, g_x1)
            sums_copy(0, 0, g_tail).wait_send()
            sums_copy(1, g_tail, groups).wait_send()

            sums_copy(3, g_late, g_late + 1).wait_recv()
            early = mine[pl.ds(g_late, 1), :] + theirs[pl.ds(g_late, 1), :]
            lane = lax.broadcasted_iota(jnp.int32, (1, _LANES), 1)
            late = jnp.zeros((1, _LANES), jnp.float32)
            late_copy().wait_recv()
            for r in range(_LATE, _TAIL_Y1[-1]):
                late = jnp.where(lane == r % _LANES, late_smem[0, r % _LANES], late)
            o_ref[pl.ds(g_late, 1), :] = early + late

    dma = pltpu.SemaphoreType.DMA
    out = pl.pallas_call(
        kernel_body,
        out_shape=jax.ShapeDtypeStruct((groups, _LANES), jnp.float32),
        in_specs=[pl.BlockSpec(memory_space=pltpu.HBM)],
        out_specs=pl.BlockSpec(memory_space=pltpu.VMEM),
        scratch_shapes=[
            pltpu.VMEM((m, n), jnp.float32),
            pltpu.VMEM((_VIA_Y[1] - _VIA_Y[0], n), jnp.float32),
            pltpu.SMEM((_VIA_SMEM[-1] - _VIA_SMEM[0], n), jnp.float32),
            pltpu.VMEM((groups, _LANES), jnp.float32),
            pltpu.VMEM((groups, _LANES), jnp.float32),
            pltpu.VMEM((g_x1 - g_x0, _LANES), jnp.float32),
            pltpu.VMEM((g_x1 - g_x0, _LANES), jnp.float32),
            pltpu.VMEM((1, _LANES), jnp.float32),
            pltpu.SMEM((1, _LANES), jnp.float32),
            dma((len(_HEAD) - 1,)),
            dma((len(_TAIL_Y1) - 1,)),
            dma((len(_VIA_SMEM) - 1,)),
            dma((len(_VIA_SMEM) - 1,)),
            dma((8,)),
            dma((8,)),
            pltpu.SemaphoreType.REGULAR,
        ],
        compiler_params=pltpu.CompilerParams(
            collective_id=0,
            vmem_limit_bytes=32 * 1024 * 1024,
            disable_bounds_checks=True,
            disable_semaphore_checks=True,
        ),
    )(x)
    return out.reshape(m, 1)
```

```python
import jax
import jax.numpy as jnp
from jax import lax
from jax.experimental import pallas as pl
from jax.experimental.pallas import tpu as pltpu

_SUBLANES = 8
_LANES = 128
_Y = 2
_UNROLL = 4

_HEAD = (0, 1024, 2048, 3072)
_TAIL_Y0 = (3072, 3840, 4096)
_TAIL_Y1 = (3072, 3328, 3488, 3512, 3528, 3536)
_LATE = _TAIL_Y1[2]
_VIA_SMEM = (3536, 3608, 3656)
_VIA_X = (3656, 3856)
_VIA_Y = (3856, 4096)


_HEAD_SUMS, _TAIL_SUMS, _X_SUMS, _EARLY_SUMS, _LATE_SUMS, _Y_ROWS, _X_ROWS, _X_BACK = range(8)


def _span(bounds, i=0, base=0):
    return pl.ds(bounds[i] - base, bounds[i + 1] - bounds[i])


def pallas_dist_mean_ax1_xy_m4096_n1024_kernel(
x: jax.Array,
):
    m, n = x.shape
    assert m == _VIA_Y[1] and n % _LANES == 0
    scale = 1.0 / (_Y * n)
    groups = m // _LANES
    g_tail = _HEAD[-1] // _LANES
    g_late = _LATE // _LANES
    g_x0, g_x1 = _VIA_X[0] // _LANES, pl.cdiv(_VIA_X[1], _LANES)
    g_y0 = _VIA_Y[0] // _LANES
    assert g_x0 == g_late + 1 and (_TAIL_Y1[-1] - 1) // _LANES == g_late

    def kernel_body(
        x_hbm, o_ref,
        x_vmem, y_vmem, x_smem, mine, theirs, x_sums, x_back, late_sums, late_smem,
        head_sems, tail_sems, smem_in_sems, smem_out_sems, send_sems, recv_sems, x_ready,
    ):
        def load(bounds, i, sems):
            rows = _span(bounds, i)
            return pltpu.make_async_copy(x_hbm.at[rows], x_vmem.at[rows], sems.at[i])

        head = [load(_HEAD, i, head_sems) for i in range(len(_HEAD) - 1)]
        head[0].start()

        my_x, my_y = lax.axis_index("x"), lax.axis_index("y")
        y_peer, x_peer = (my_x, 1 - my_y), (1 - my_x, my_y)
        barrier = pltpu.get_barrier_semaphore()

        def signal(sem, peer):
            pl.semaphore_signal(sem, inc=1, device_id=peer, device_id_type=pl.DeviceIdType.MESH)

        signal(barrier, y_peer)

        def remote(src, dst, i, peer):
            return pltpu.make_async_remote_copy(
                src, dst, send_sems.at[i], recv_sems.at[i],
                device_id=peer, device_id_type=pl.DeviceIdType.MESH)

        def sums_copy(i, g0, g1):
            rows = pl.ds(g0, g1 - g0)
            return remote(mine.at[rows], theirs.at[rows], i, y_peer)

        def late_copy():
            return remote(late_sums, late_smem, _LATE_SUMS, y_peer)

        def rows_to_y_peer():
            return remote(x_hbm.at[_span(_VIA_Y)], y_vmem, _Y_ROWS, y_peer)

        def rows_to_x_peer():
            return remote(x_hbm.at[_span(_VIA_X)], x_vmem.at[_span(_VIA_X)], _X_ROWS, x_peer)

        def sums_to_x_peer():
            return remote(x_sums, x_back, _X_BACK, x_peer)

        def smem_in(i):
            return pltpu.make_async_copy(
                x_hbm.at[_span(_VIA_SMEM, i)], x_smem.at[_span(_VIA_SMEM, i, _VIA_SMEM[0])],
                smem_in_sems.at[i])

        def smem_out(i):
            return pltpu.make_async_copy(
                x_smem.at[_span(_VIA_SMEM, i, _VIA_SMEM[0])], x_vmem.at[_span(_VIA_SMEM, i)],
                smem_out_sems.at[i])

        tile = (_SUBLANES, _LANES)
        diagonal = lax.broadcasted_iota(jnp.int32, tile, 1) - lax.broadcasted_iota(jnp.int32, tile, 0)
        zero = jnp.zeros(tile, jnp.float32)

        def fold(ref, r):
            v = [ref[pl.ds(r, _SUBLANES), pl.ds(c, _LANES)] for c in range(0, n, _LANES)]
            while len(v) > 1:
                v = [v[i] + v[i + 1] for i in range(0, len(v) - 1, 2)] + v[len(v) // 2 * 2:]
            return v[0]

        def place(acc, r, folded):
            return jnp.where(diagonal == r % _LANES, jnp.sum(folded, axis=1, keepdims=True), acc)

        def add_rows(acc, ref, r0, r1, offset=0):
            for r in range(r0, r1, _SUBLANES):
                acc = place(acc, r, fold(ref, offset + r))
            return acc

        def dense(acc):
            return jnp.sum(acc, axis=0, keepdims=True) * scale

        def overlap(g, r0, r1):
            return max(r0, g * _LANES), min(r1, (g + 1) * _LANES)

        def sum_groups(g0, g1):
            steps = (g1 - g0) // _UNROLL
            looped = steps * _UNROLL if steps > 1 else 0
            if looped:
                @pl.loop(0, steps)
                def _(i):
                    for u in range(_UNROLL):
                        g = g0 + i * _UNROLL + u
                        start = pl.multiple_of(g * _LANES, _LANES)
                        mine[pl.ds(g, 1), :] = dense(add_rows(zero, x_vmem, 0, _LANES, start))
            for g in range(g0 + looped, g1):
                mine[pl.ds(g, 1), :] = dense(add_rows(zero, x_vmem, 0, _LANES, g * _LANES))

        def finish(copy_index, g0, g1):
            sums_copy(copy_index, g0, g1).wait_recv()
            rows = pl.ds(g0, g1 - g0)
            o_ref[rows, :] = mine[rows, :] + theirs[rows, :]

        @pl.when(my_y == 1)
        def _():
            smem_in(0).start()

            @pl.when(my_x == 0)
            def _():
                signal(barrier, x_peer)
                pl.semaphore_wait(barrier, 1)

            @pl.when(my_x == 1)
            def _():
                pl.semaphore_wait(barrier, 2)
                signal(x_ready, x_peer)

            rows_to_y_peer().start()
            for copy in head[1:]:
                copy.start()
            for i in range(len(_TAIL_Y1) - 1):
                load(_TAIL_Y1, i, tail_sems).start()

            @pl.when(my_x == 0)
            def _():
                pl.semaphore_wait(x_ready, 1)

            rows_to_x_peer().start()

        @pl.when(my_y == 0)
        def _():
            for copy in head[1:]:
                copy.start()
            for i in range(len(_TAIL_Y0) - 1):
                load(_TAIL_Y0, i, tail_sems).start()
            pl.semaphore_wait(barrier, 1)

        smem_steps = len(_VIA_SMEM) - 1
        for i, copy in enumerate(head):
            copy.wait()
            if i < smem_steps:
                @pl.when(my_y == 1)
                def _():
                    smem_in(i).wait()
                    smem_out(i).start()
                    if i + 1 < smem_steps:
                        smem_in(i + 1).start()
            sum_groups(_HEAD[i] // _LANES, _HEAD[i + 1] // _LANES)
        sums_copy(_HEAD_SUMS, 0, g_tail).start()

        @pl.when(my_y == 1)
        def _():
            rows_to_x_peer().wait_recv()
            for g in range(g_x0, g_x1):
                x_sums[pl.ds(g - g_x0, 1), :] = dense(add_rows(zero, x_vmem, *overlap(g, *_VIA_X)))
            sums_to_x_peer().start()

            load(_TAIL_Y1, 0, tail_sems).wait()
            sum_groups(g_tail, _TAIL_Y1[1] // _LANES)

            for i in range(smem_steps):
                smem_out(i).wait()
            acc = add_rows(zero, x_vmem, *overlap(g_late, _VIA_SMEM[0], _VIA_SMEM[-1]))
            for g in range(g_late + 1, groups):
                rows = overlap(g, _VIA_SMEM[0], _VIA_SMEM[-1])
                mine[pl.ds(g, 1), :] = dense(add_rows(zero, x_vmem, *rows))

            load(_TAIL_Y1, 1, tail_sems).wait()
            sum_groups(_TAIL_Y1[1] // _LANES, g_late)
            acc = add_rows(acc, x_vmem, g_late * _LANES, _LATE)
            sums_copy(_TAIL_SUMS, g_tail, g_late).start()
            mine[pl.ds(g_late, 1), :] = dense(acc)
            sums_copy(_EARLY_SUMS, g_late, g_late + 1).start()

            sums_to_x_peer().wait_recv()
            mine[pl.ds(g_x0, g_x1 - g_x0), :] += x_back[...]
            sums_copy(_X_SUMS, g_x0, g_x1).start()

            folded = []
            for i in range(2, len(_TAIL_Y1) - 1):
                load(_TAIL_Y1, i, tail_sems).wait()
                folded += [(r, fold(x_vmem, r)) for r in range(_TAIL_Y1[i], _TAIL_Y1[i + 1], _SUBLANES)]
            acc = zero
            for r, v in folded:
                acc = place(acc, r, v)
            late_sums[...] = dense(acc)
            late_copy().start()

            for copy in (
                rows_to_y_peer(), rows_to_x_peer(), sums_to_x_peer(), late_copy(),
                sums_copy(_HEAD_SUMS, 0, g_tail), sums_copy(_TAIL_SUMS, g_tail, g_late),
                sums_copy(_X_SUMS, g_x0, g_x1), sums_copy(_EARLY_SUMS, g_late, g_late + 1),
            ):
                copy.wait_send()
            finish(_HEAD_SUMS, 0, g_tail)
            finish(_TAIL_SUMS, g_tail, groups)
            o_ref[pl.ds(g_late, 1), :] += late_sums[...]

        @pl.when(my_y == 0)
        def _():
            for i in range(len(_TAIL_Y0) - 1):
                load(_TAIL_Y0, i, tail_sems).wait()
                sum_groups(_TAIL_Y0[i] // _LANES, _TAIL_Y0[i + 1] // _LANES)

            rows_to_y_peer().wait_recv()
            for g in range(g_y0, groups):
                mine[pl.ds(g, 1), :] += dense(add_rows(zero, y_vmem, *overlap(g, *_VIA_Y), -_VIA_Y[0]))
            sums_copy(_TAIL_SUMS, g_tail, groups).start()

            o_ref[pl.ds(g_x1, groups - g_x1), :] = mine[pl.ds(g_x1, groups - g_x1), :]
            finish(_HEAD_SUMS, 0, g_tail)
            finish(_TAIL_SUMS, g_tail, g_late)
            finish(_X_SUMS, g_x0, g_x1)
            sums_copy(_HEAD_SUMS, 0, g_tail).wait_send()
            sums_copy(_TAIL_SUMS, g_tail, groups).wait_send()

            sums_copy(_EARLY_SUMS, g_late, g_late + 1).wait_recv()
            early = mine[pl.ds(g_late, 1), :] + theirs[pl.ds(g_late, 1), :]
            lane = lax.broadcasted_iota(jnp.int32, (1, _LANES), 1)
            late = jnp.zeros((1, _LANES), jnp.float32)
            late_copy().wait_recv()
            for r in range(_LATE, _TAIL_Y1[-1]):
                late = jnp.where(lane == r % _LANES, late_smem[0, r % _LANES], late)
            o_ref[pl.ds(g_late, 1), :] = early + late

    dma = pltpu.SemaphoreType.DMA
    out = pl.pallas_call(
        kernel_body,
        out_shape=jax.ShapeDtypeStruct((groups, _LANES), jnp.float32),
        in_specs=[pl.BlockSpec(memory_space=pltpu.HBM)],
        out_specs=pl.BlockSpec(memory_space=pltpu.VMEM),
        scratch_shapes=[
            pltpu.VMEM((m, n), jnp.float32),
            pltpu.VMEM((_VIA_Y[1] - _VIA_Y[0], n), jnp.float32),
            pltpu.SMEM((_VIA_SMEM[-1] - _VIA_SMEM[0], n), jnp.float32),
            pltpu.VMEM((groups, _LANES), jnp.float32),
            pltpu.VMEM((groups, _LANES), jnp.float32),
            pltpu.VMEM((g_x1 - g_x0, _LANES), jnp.float32),
            pltpu.VMEM((g_x1 - g_x0, _LANES), jnp.float32),
            pltpu.VMEM((1, _LANES), jnp.float32),
            pltpu.SMEM((1, _LANES), jnp.float32),
            dma((len(_HEAD) - 1,)),
            dma((len(_TAIL_Y1) - 1,)),
            dma((len(_VIA_SMEM) - 1,)),
            dma((len(_VIA_SMEM) - 1,)),
            dma((_X_BACK + 1,)),
            dma((_X_BACK + 1,)),
            pltpu.SemaphoreType.REGULAR,
        ],
        compiler_params=pltpu.CompilerParams(
            collective_id=0,
            vmem_limit_bytes=32 * 1024 * 1024,
            disable_bounds_checks=True,
            disable_semaphore_checks=True,
        ),
    )(x)
    return out.reshape(m, 1)
```
